```python
import numpy as np

kernel_name = "dist_mean_ax0_shard0_i_m1024_n512"

def setup_inputs():
    return {"x": np.random.randn(4096, 512).astype(np.float32)}

def reference(x: np.ndarray) -> np.ndarray:
    return np.mean(x, axis=0, keepdims=True)
```

```python
import jax
import jax.numpy as jnp
from jax import lax
from jax.experimental import pallas as pl
from jax.experimental.pallas import tpu as pltpu

N_DEV = 4
LATE = 2
GIFT_ROWS = 40
TAIL_ROWS = 96
LAST_CHUNK_ROWS = 256
NARROW_COLS = 128
SUBLANES = 8


def _add_rows(ref, row0, rows, acc, chains):
    accs = [acc] + [None] * (chains - 1)
    for t in range(rows // SUBLANES):
        tile = ref[pl.ds(row0 + t * SUBLANES, SUBLANES), :]
        k = (t + 1) % chains
        accs[k] = tile if accs[k] is None else accs[k] + tile
    accs = [a for a in accs if a is not None]
    while len(accs) > 1:
        pairs = [accs[i : i + 2] for i in range(0, len(accs), 2)]
        accs = [p[0] + p[1] if len(p) == 2 else p[0] for p in pairs]
    return accs[0]


def pallas_dist_mean_ax0_shard0_i_m1024_n512_kernel(
    x: jax.Array,
):
    m, n = x.shape
    tail0 = m - TAIL_ROWS
    last0 = tail0 - LAST_CHUNK_ROWS
    chunks = ((2 * GIFT_ROWS, last0 - 2 * GIFT_ROWS), (last0, LAST_CHUNK_ROWS))
    groups = ((0, n - NARROW_COLS), (n - NARROW_COLS, NARROW_COLS))

    def kernel_body(
        x_hbm,
        o_ref,
        rows_buf,
        wide_buf,
        narrow_buf,
        gift_buf,
        acc_buf,
        mine,
        near,
        far,
        chunk_sems,
        tail_sems,
        head_sem,
        gift_send_sems,
        gift_recv_sem,
        near_send_sems,
        near_recv_sem,
        far_send_sems,
        far_recv_sem,
    ):
        chunk_loads = [
            pltpu.make_async_copy(
                x_hbm.at[pl.ds(row0, rows)],
                rows_buf.at[pl.ds(row0, rows)],
                chunk_sems.at[c],
            )
            for c, (row0, rows) in enumerate(chunks)
        ]
        tail_bufs = (wide_buf, narrow_buf)
        tail_loads = [
            pltpu.make_async_copy(
                x_hbm.at[pl.ds(tail0, TAIL_ROWS), pl.ds(col0, cols)],
                tail_bufs[g],
                tail_sems.at[g],
            )
            for g, (col0, cols) in enumerate(groups)
        ]
        for load in chunk_loads + tail_loads:
            load.start()

        me = lax.axis_index("i")
        is_late = me == LATE
        is_late_neighbour = (me & 1) != (LATE & 1)
        peers = [(me + d) & (N_DEV - 1) for d in range(N_DEV)]

        head_load = pltpu.make_async_copy(
            x_hbm.at[pl.ds(0, 2 * GIFT_ROWS)],
            rows_buf.at[pl.ds(0, 2 * GIFT_ROWS)],
            head_sem,
        )

        @pl.when(jnp.logical_not(is_late))
        def _():
            head_load.start()

        barrier_sem = pltpu.get_barrier_semaphore()
        for d in range(1, N_DEV):
            pl.semaphore_signal(
                barrier_sem,
                inc=1,
                device_id=(peers[d],),
                device_id_type=pl.DeviceIdType.MESH,
            )
        pl.semaphore_wait(barrier_sem, N_DEV - 1)

        def gift_copy(k):
            return pltpu.make_async_remote_copy(
                src_ref=x_hbm.at[pl.ds(k * GIFT_ROWS, GIFT_ROWS)],
                dst_ref=gift_buf,
                send_sem=gift_send_sems.at[k],
                recv_sem=gift_recv_sem,
                device_id=((LATE + 2 * k + 1) % N_DEV,),
                device_id_type=pl.DeviceIdType.MESH,
            )

        @pl.when(is_late)
        def _():
            gift_copy(0).start()
            gift_copy(1).start()

        acc = None
        for load, (row0, rows) in zip(chunk_loads, chunks):
            load.wait()
            acc = _add_rows(rows_buf, row0, rows, acc, chains=2)
        acc_buf[...] = acc

        @pl.when(jnp.logical_not(is_late))
        def _():
            head_load.wait()
            acc_buf[...] = _add_rows(
                rows_buf, 0, 2 * GIFT_ROWS, acc_buf[...], chains=2
            )

        @pl.when(is_late_neighbour)
        def _():
            gift_copy(0).wait_recv()
            acc_buf[...] = _add_rows(gift_buf, 0, GIFT_ROWS, acc_buf[...], chains=2)

        acc = acc_buf[...]

        sends = []
        for g, (col0, cols) in enumerate(groups):
            tail_loads[g].wait()
            sums = _add_rows(
                tail_bufs[g], 0, TAIL_ROWS, acc[:, col0 : col0 + cols], chains=4
            )
            mine[:, pl.ds(col0, cols)] = jnp.sum(sums, axis=0, keepdims=True)
            sends.append(
                pltpu.make_async_remote_copy(
                    src_ref=mine.at[:, pl.ds(col0, cols)],
                    dst_ref=far.at[:, pl.ds(col0, cols)],
                    send_sem=far_send_sems.at[g],
                    recv_sem=far_recv_sem,
                    device_id=(peers[2],),
                    device_id_type=pl.DeviceIdType.MESH,
                )
            )
            sends[-1].start()

        for k, d in enumerate((1, 3)):
            sends.append(
                pltpu.make_async_remote_copy(
                    src_ref=mine,
                    dst_ref=near.at[k],
                    send_sem=near_send_sems.at[k],
                    recv_sem=near_recv_sem,
                    device_id=(peers[d],),
                    device_id_type=pl.DeviceIdType.MESH,
                )
            )
            sends[-1].start()

        for send in sends:
            send.wait_send()

        @pl.when(is_late)
        def _():
            gift_copy(0).wait_send()
            gift_copy(1).wait_send()

        pltpu.make_async_copy(near, near, near_recv_sem).wait()
        near_sum = near[0] + near[1]
        own = mine[...]
        pltpu.make_async_copy(far, far, far_recv_sem).wait()
        o_ref[...] = ((own + far[...]) + near_sum) * (1.0 / (m * N_DEV))

    return pl.pallas_call(
        kernel_body,
        out_shape=jax.ShapeDtypeStruct((1, n), jnp.float32),
        in_specs=[pl.BlockSpec(memory_space=pl.ANY)],
        out_specs=pl.BlockSpec(memory_space=pltpu.VMEM),
        scratch_shapes=[
            pltpu.VMEM((m, n), jnp.float32),
            pltpu.VMEM((TAIL_ROWS, n - NARROW_COLS), jnp.float32),
            pltpu.VMEM((TAIL_ROWS, NARROW_COLS), jnp.float32),
            pltpu.VMEM((GIFT_ROWS, n), jnp.float32),
            pltpu.VMEM((SUBLANES, n), jnp.float32),
            pltpu.VMEM((1, n), jnp.float32),
            pltpu.VMEM((2, 1, n), jnp.float32),
            pltpu.VMEM((1, n), jnp.float32),
            pltpu.SemaphoreType.DMA((len(chunks),)),
            pltpu.SemaphoreType.DMA((len(groups),)),
            pltpu.SemaphoreType.DMA,
            pltpu.SemaphoreType.DMA((2,)),
            pltpu.SemaphoreType.DMA,
            pltpu.SemaphoreType.DMA((2,)),
            pltpu.SemaphoreType.DMA,
            pltpu.SemaphoreType.DMA((len(groups),)),
            pltpu.SemaphoreType.DMA,
        ],
        compiler_params=pltpu.CompilerParams(
            collective_id=0,
            disable_semaphore_checks=True,
        ),
    )(x)
```

```python
import jax
import jax.numpy as jnp
from jax import lax
from jax.experimental import pallas as pl
from jax.experimental.pallas import tpu as pltpu

N_DEV = 4
SUBLANES = 8
LATE = 2

FULL_CHUNKS = (400, 192, 128)
NARROW_CHUNKS = (192, 32)
TAIL_ROWS = sum(NARROW_CHUNKS)
GIFT_ROWS = 40
NARROW_COLS = 128


def _add_rows(acc, ref, row0, rows, chains):
    accs = [acc] + [None] * (chains - 1)
    for t in range(rows // SUBLANES):
        tile = ref[pl.ds(row0 + t * SUBLANES, SUBLANES), :]
        k = (t + 1) % chains
        accs[k] = tile if accs[k] is None else accs[k] + tile
    accs = [a for a in accs if a is not None]
    while len(accs) > 1:
        pairs = [accs[i : i + 2] for i in range(0, len(accs), 2)]
        accs = [p[0] + p[1] if len(p) == 2 else p[0] for p in pairs]
    return accs[0]


def _offsets(sizes):
    return [sum(sizes[:k]) for k in range(len(sizes))]


def pallas_dist_mean_ax0_shard0_i_m1024_n512_kernel(
    x: jax.Array,
):
    m, n = x.shape
    wide_cols = n - NARROW_COLS
    tail0 = sum(FULL_CHUNKS)
    spare0 = tail0 + TAIL_ROWS
    assert spare0 + 2 * GIFT_ROWS == m
    full_chunks = list(zip(_offsets(FULL_CHUNKS), FULL_CHUNKS))
    narrow_chunks = list(zip(_offsets(NARROW_CHUNKS), NARROW_CHUNKS))
    n_loads = len(full_chunks) + len(narrow_chunks) + 2

    def kernel_body(
        x_hbm,
        o_ref,
        full_buf,
        wide_buf,
        narrow_buf,
        spare_buf,
        gift_buf,
        acc_buf,
        mine,
        near,
        far,
        load_sems,
        gift_send_sems,
        gift_recv_sem,
        near_send_sems,
        near_recv_sem,
        far_send_sems,
        far_recv_sem,
    ):
        sems = iter([load_sems.at[k] for k in range(n_loads)])
        full_loads = [
            pltpu.make_async_copy(
                x_hbm.at[pl.ds(row0, rows)], full_buf.at[pl.ds(row0, rows)], next(sems)
            )
            for row0, rows in full_chunks
        ]
        wide_load = pltpu.make_async_copy(
            x_hbm.at[pl.ds(tail0, TAIL_ROWS), pl.ds(0, wide_cols)],
            wide_buf,
            next(sems),
        )
        narrow_loads = [
            pltpu.make_async_copy(
                x_hbm.at[pl.ds(tail0 + row0, rows), pl.ds(wide_cols, NARROW_COLS)],
                narrow_buf.at[pl.ds(row0, rows)],
                next(sems),
            )
            for row0, rows in narrow_chunks
        ]
        spare_load = pltpu.make_async_copy(
            x_hbm.at[pl.ds(spare0, 2 * GIFT_ROWS)], spare_buf, next(sems)
        )
        for load in [full_loads[0], wide_load, *full_loads[1:], *narrow_loads]:
            load.start()

        me = lax.axis_index("i")
        is_late = me == LATE
        is_late_neighbour = (me & 1) != (LATE & 1)
        peers = [(me + d) & (N_DEV - 1) for d in range(N_DEV)]

        @pl.when(jnp.logical_not(is_late))
        def _():
            spare_load.start()

        barrier_sem = pltpu.get_barrier_semaphore()
        for d in range(1, N_DEV):
            pl.semaphore_signal(
                barrier_sem,
                inc=1,
                device_id=(peers[d],),
                device_id_type=pl.DeviceIdType.MESH,
            )
        pl.semaphore_wait(barrier_sem, N_DEV - 1)

        def gift_copy(k):
            return pltpu.make_async_remote_copy(
                src_ref=x_hbm.at[pl.ds(spare0 + k * GIFT_ROWS, GIFT_ROWS)],
                dst_ref=gift_buf,
                send_sem=gift_send_sems.at[k],
                recv_sem=gift_recv_sem,
                device_id=((LATE + 2 * k + 1) % N_DEV,),
                device_id_type=pl.DeviceIdType.MESH,
            )

        @pl.when(is_late)
        def _():
            gift_copy(0).start()
            gift_copy(1).start()

        full_loads[0].wait()
        acc = _add_rows(None, full_buf, *full_chunks[0], chains=2)
        wide_load.wait()
        wide_acc = _add_rows(acc[:, :wide_cols], wide_buf, 0, TAIL_ROWS, chains=3)
        acc = jnp.concatenate([wide_acc, acc[:, wide_cols:]], axis=1)
        for load, (row0, rows) in zip(full_loads[1:-1], full_chunks[1:-1]):
            load.wait()
            acc = _add_rows(acc, full_buf, row0, rows, chains=2)
        acc_buf[...] = acc

        @pl.when(jnp.logical_not(is_late))
        def _():
            spare_load.wait()
            acc_buf[...] = _add_rows(
                acc_buf[...], spare_buf, 0, 2 * GIFT_ROWS, chains=2
            )

        @pl.when(is_late_neighbour)
        def _():
            gift_copy(0).wait_recv()
            acc_buf[...] = _add_rows(acc_buf[...], gift_buf, 0, GIFT_ROWS, chains=2)

        acc = acc_buf[...]
        full_loads[-1].wait()
        acc = _add_rows(acc, full_buf, *full_chunks[-1], chains=2)

        def send_far(k, col0, cols, sums):
            mine[:, pl.ds(col0, cols)] = jnp.sum(sums, axis=0, keepdims=True)
            copy = pltpu.make_async_remote_copy(
                src_ref=mine.at[:, pl.ds(col0, cols)],
                dst_ref=far.at[:, pl.ds(col0, cols)],
                send_sem=far_send_sems.at[k],
                recv_sem=far_recv_sem,
                device_id=(peers[2],),
                device_id_type=pl.DeviceIdType.MESH,
            )
            copy.start()
            return copy

        sends = [send_far(0, 0, wide_cols, acc[:, :wide_cols])]
        narrow_acc = acc[:, wide_cols:]
        for load, (row0, rows) in zip(narrow_loads, narrow_chunks):
            load.wait()
            narrow_acc = _add_rows(narrow_acc, narrow_buf, row0, rows, chains=8)
        sends.append(send_far(1, wide_cols, NARROW_COLS, narrow_acc))

        for k, d in enumerate((1, 3)):
            copy = pltpu.make_async_remote_copy(
                src_ref=mine,
                dst_ref=near.at[k],
                send_sem=near_send_sems.at[k],
                recv_sem=near_recv_sem,
                device_id=(peers[d],),
                device_id_type=pl.DeviceIdType.MESH,
            )
            copy.start()
            sends.append(copy)

        for copy in sends:
            copy.wait_send()

        @pl.when(is_late)
        def _():
            gift_copy(0).wait_send()
            gift_copy(1).wait_send()

        pltpu.make_async_copy(near, near, near_recv_sem).wait()
        near_sum = near[0] + near[1]
        own = mine[...]
        pltpu.make_async_copy(far, far, far_recv_sem).wait()
        o_ref[...] = ((own + far[...]) + near_sum) * (1.0 / (m * N_DEV))

    return pl.pallas_call(
        kernel_body,
        out_shape=jax.ShapeDtypeStruct((1, n), jnp.float32),
        in_specs=[pl.BlockSpec(memory_space=pl.ANY)],
        out_specs=pl.BlockSpec(memory_space=pltpu.VMEM),
        scratch_shapes=[
            pltpu.VMEM((tail0, n), jnp.float32),
            pltpu.VMEM((TAIL_ROWS, wide_cols), jnp.float32),
            pltpu.VMEM((TAIL_ROWS, NARROW_COLS), jnp.float32),
            pltpu.VMEM((2 * GIFT_ROWS, n), jnp.float32),
            pltpu.VMEM((GIFT_ROWS, n), jnp.float32),
            pltpu.VMEM((SUBLANES, n), jnp.float32),
            pltpu.VMEM((1, n), jnp.float32),
            pltpu.VMEM((2, 1, n), jnp.float32),
            pltpu.VMEM((1, n), jnp.float32),
            pltpu.SemaphoreType.DMA((n_loads,)),
            pltpu.SemaphoreType.DMA((2,)),
            pltpu.SemaphoreType.DMA,
            pltpu.SemaphoreType.DMA((2,)),
            pltpu.SemaphoreType.DMA,
            pltpu.SemaphoreType.DMA((2,)),
            pltpu.SemaphoreType.DMA,
        ],
        compiler_params=pltpu.CompilerParams(
            collective_id=0,
            disable_semaphore_checks=True,
        ),
    )(x)
```

```python
import jax
import jax.numpy as jnp
from jax import lax
from jax.experimental import pallas as pl
from jax.experimental.pallas import tpu as pltpu

N_DEV = 4
SUBLANES = 8
LATE = 2

FULL_CHUNKS = (400, 192, 128)
NARROW_CHUNKS = (192, 32)
TAIL_ROWS = sum(NARROW_CHUNKS)
GIFT_ROWS = 40
NARROW_COLS = 128


def _add_rows(acc, ref, row0, rows, chains):
    accs = [acc] + [None] * (chains - 1)
    for t in range(rows // SUBLANES):
        tile = ref[pl.ds(row0 + t * SUBLANES, SUBLANES), :]
        k = (t + 1) % chains
        accs[k] = tile if accs[k] is None else accs[k] + tile
    accs = [a for a in accs if a is not None]
    while len(accs) > 1:
        pairs = [accs[i : i + 2] for i in range(0, len(accs), 2)]
        accs = [p[0] + p[1] if len(p) == 2 else p[0] for p in pairs]
    return accs[0]


def _offsets(sizes):
    return [sum(sizes[:k]) for k in range(len(sizes))]


def pallas_dist_mean_ax0_shard0_i_m1024_n512_kernel(
    x: jax.Array,
):
    m, n = x.shape
    wide_cols = n - NARROW_COLS
    tail0 = sum(FULL_CHUNKS)
    spare0 = tail0 + TAIL_ROWS
    assert spare0 + 2 * GIFT_ROWS == m
    full_chunks = list(zip(_offsets(FULL_CHUNKS), FULL_CHUNKS))
    narrow_chunks = list(zip(_offsets(NARROW_CHUNKS), NARROW_CHUNKS))
    n_loads = len(full_chunks) + len(narrow_chunks) + 2

    def kernel_body(
        x_hbm,
        o_ref,
        full_buf,
        wide_buf,
        narrow_buf,
        spare_buf,
        gift_buf,
        acc_buf,
        mine,
        near,
        far,
        load_sems,
        gift_send_sems,
        gift_recv_sem,
        near_send_sems,
        near_recv_sem,
        far_send_sems,
        far_recv_sem,
    ):
        sems = iter([load_sems.at[k] for k in range(n_loads)])
        full_loads = [
            pltpu.make_async_copy(
                x_hbm.at[pl.ds(row0, rows)], full_buf.at[pl.ds(row0, rows)], next(sems)
            )
            for row0, rows in full_chunks
        ]
        wide_load = pltpu.make_async_copy(
            x_hbm.at[pl.ds(tail0, TAIL_ROWS), pl.ds(0, wide_cols)],
            wide_buf,
            next(sems),
        )
        narrow_loads = [
            pltpu.make_async_copy(
                x_hbm.at[pl.ds(tail0 + row0, rows), pl.ds(wide_cols, NARROW_COLS)],
                narrow_buf.at[pl.ds(row0, rows)],
                next(sems),
            )
            for row0, rows in narrow_chunks
        ]
        spare_load = pltpu.make_async_copy(
            x_hbm.at[pl.ds(spare0, 2 * GIFT_ROWS)], spare_buf, next(sems)
        )
        for load in [full_loads[0], wide_load, *full_loads[1:], *narrow_loads]:
            load.start()

        me = lax.axis_index("i")
        is_late = me == LATE
        is_late_neighbour = (me & 1) != (LATE & 1)
        peers = [(me + d) & (N_DEV - 1) for d in range(N_DEV)]

        @pl.when(jnp.logical_not(is_late))
        def _():
            spare_load.start()

        barrier_sem = pltpu.get_barrier_semaphore()
        for d in range(1, N_DEV):
            pl.semaphore_signal(
                barrier_sem,
                inc=1,
                device_id=(peers[d],),
                device_id_type=pl.DeviceIdType.MESH,
            )
        pl.semaphore_wait(barrier_sem, N_DEV - 1)

        def gift_copy(k, peer):
            return pltpu.make_async_remote_copy(
                src_ref=x_hbm.at[pl.ds(spare0 + k * GIFT_ROWS, GIFT_ROWS)],
                dst_ref=gift_buf,
                send_sem=gift_send_sems.at[k],
                recv_sem=gift_recv_sem,
                device_id=(peer,),
                device_id_type=pl.DeviceIdType.MESH,
            )

        gifts = [gift_copy(k, (LATE + d) % N_DEV) for k, d in enumerate((1, 3))]

        @pl.when(is_late)
        def _():
            for gift in gifts:
                gift.start()

        full_loads[0].wait()
        acc = _add_rows(None, full_buf, *full_chunks[0], chains=2)
        wide_load.wait()
        wide_acc = _add_rows(acc[:, :wide_cols], wide_buf, 0, TAIL_ROWS, chains=3)
        acc = jnp.concatenate([wide_acc, acc[:, wide_cols:]], axis=1)
        for load, (row0, rows) in zip(full_loads[1:-1], full_chunks[1:-1]):
            load.wait()
            acc = _add_rows(acc, full_buf, row0, rows, chains=2)
        acc_buf[...] = acc

        @pl.when(jnp.logical_not(is_late))
        def _():
            spare_load.wait()
            acc_buf[...] = _add_rows(
                acc_buf[...], spare_buf, 0, 2 * GIFT_ROWS, chains=2
            )

        @pl.when(is_late_neighbour)
        def _():
            gift_copy(0, LATE).wait_recv()
            acc_buf[...] = _add_rows(acc_buf[...], gift_buf, 0, GIFT_ROWS, chains=2)

        acc = acc_buf[...]
        full_loads[-1].wait()
        acc = _add_rows(acc, full_buf, *full_chunks[-1], chains=2)

        def send_far(k, col0, cols, sums):
            mine[:, pl.ds(col0, cols)] = jnp.sum(sums, axis=0, keepdims=True)
            copy = pltpu.make_async_remote_copy(
                src_ref=mine.at[:, pl.ds(col0, cols)],
                dst_ref=far.at[:, pl.ds(col0, cols)],
                send_sem=far_send_sems.at[k],
                recv_sem=far_recv_sem,
                device_id=(peers[2],),
                device_id_type=pl.DeviceIdType.MESH,
            )
            copy.start()
            return copy

        sends = [send_far(0, 0, wide_cols, acc[:, :wide_cols])]
        narrow_acc = acc[:, wide_cols:]
        for load, (row0, rows) in zip(narrow_loads, narrow_chunks):
            load.wait()
            narrow_acc = _add_rows(narrow_acc, narrow_buf, row0, rows, chains=8)
        sends.append(send_far(1, wide_cols, NARROW_COLS, narrow_acc))

        for k, d in enumerate((1, 3)):
            copy = pltpu.make_async_remote_copy(
                src_ref=mine,
                dst_ref=near.at[k],
                send_sem=near_send_sems.at[k],
                recv_sem=near_recv_sem,
                device_id=(peers[d],),
                device_id_type=pl.DeviceIdType.MESH,
            )
            copy.start()
            sends.append(copy)

        for copy in sends:
            copy.wait_send()

        @pl.when(is_late)
        def _():
            for gift in gifts:
                gift.wait_send()

        pltpu.make_async_copy(near, near, near_recv_sem).wait()
        near_sum = near[0] + near[1]
        own = mine[...]
        pltpu.make_async_copy(far, far, far_recv_sem).wait()
        o_ref[...] = ((own + far[...]) + near_sum) * (1.0 / (m * N_DEV))

    return pl.pallas_call(
        kernel_body,
        out_shape=jax.ShapeDtypeStruct((1, n), jnp.float32),
        in_specs=[pl.BlockSpec(memory_space=pl.ANY)],
        out_specs=pl.BlockSpec(memory_space=pltpu.VMEM),
        scratch_shapes=[
            pltpu.VMEM((tail0, n), jnp.float32),
            pltpu.VMEM((TAIL_ROWS, wide_cols), jnp.float32),
            pltpu.VMEM((TAIL_ROWS, NARROW_COLS), jnp.float32),
            pltpu.VMEM((2 * GIFT_ROWS, n), jnp.float32),
            pltpu.VMEM((GIFT_ROWS, n), jnp.float32),
            pltpu.VMEM((SUBLANES, n), jnp.float32),
            pltpu.VMEM((1, n), jnp.float32),
            pltpu.VMEM((2, 1, n), jnp.float32),
            pltpu.VMEM((1, n), jnp.float32),
            pltpu.SemaphoreType.DMA((n_loads,)),
            pltpu.SemaphoreType.DMA((2,)),
            pltpu.SemaphoreType.DMA,
            pltpu.SemaphoreType.DMA((2,)),
            pltpu.SemaphoreType.DMA,
            pltpu.SemaphoreType.DMA((2,)),
            pltpu.SemaphoreType.DMA,
        ],
        compiler_params=pltpu.CompilerParams(
            collective_id=0,
            disable_semaphore_checks=True,
        ),
    )(x)
```
